```python
import numpy as np

kernel_name = "dist_moe_cap_ep_outshard_n2048_d512_e8_h1024"

def setup_inputs():
    x = np.random.randn(2048, 512).astype(np.float32)
    router_W = np.random.randn(512, 32).astype(np.float32) * 0.1
    scores64 = x.astype(np.float64) @ router_W.astype(np.float64)
    route_idx = np.argsort(-scores64, axis=-1)[:, :1].astype(np.int32)
    expert_W = np.random.randn(32, 512, 1024).astype(np.float32) * 0.02
    return {"x": x, "router_W": router_W, "route_idx": route_idx, "expert_W": expert_W}

def reference(x, router_W, route_idx, expert_W):
    counts = np.zeros(32, dtype=np.int64)
    out = np.zeros((2048, 1024), dtype=np.float32)
    for i in range(2048):
        e = int(route_idx[i, 0])
        if counts[e] < 51:
            out[i] = x[i] @ expert_W[e]
            counts[e] += 1
    return out
```

```python
import jax
import jax.numpy as jnp
from jax import lax
from jax.experimental import pallas as pl
from jax.experimental.pallas import tpu as pltpu

N_DEV = 4
N_TOK = 2048
D = 512
H = 1024
E_LOC = 8
CAP = 51
CPAD = 64
ROWS = N_TOK // N_DEV


def _body(x_ref, ri_ref, w_ref, o_ref,
          wbuf, xg, y, rbuf, meta_v, meta_s, zrow, stage,
          wsem, gsem, msem, ssem, rsem):
    me = lax.axis_index("i")
    bar = pltpu.get_barrier_semaphore()
    for k in range(1, N_DEV):
        pl.semaphore_signal(bar, inc=1, device_id=(me + k) % N_DEV,
                            device_id_type=pl.DeviceIdType.LOGICAL)

    rcp = pltpu.make_async_copy(ri_ref, rbuf, msem)
    rcp.start()
    wcps = [pltpu.make_async_copy(w_ref.at[e], wbuf.at[e], wsem.at[e])
            for e in range(E_LOC)]
    for cp in wcps:
        cp.start(priority=1)
    zrow[...] = jnp.zeros_like(zrow)
    rcp.wait()

    f32, bf16 = jnp.float32, jnp.bfloat16
    R = rbuf[...]
    ri = lax.broadcasted_iota(jnp.int32, (128, 128), 0)
    ci = lax.broadcasted_iota(jnp.int32, (128, 128), 1)
    U = (ri <= ci).astype(bf16)
    ONES = jnp.ones((128, 128), bf16)
    L = ((ci < ri) & ((ci >> 4) == (ri >> 4))).astype(bf16)
    R8 = jnp.concatenate([R] * 8, axis=0)
    le_row = ri >> 4

    def dot(a, b):
        return jnp.dot(a, b, preferred_element_type=f32)

    rank = jnp.zeros((16, 128), f32)
    for g in range(N_DEV):
        base = ((me + g) % N_DEV) * E_LOC
        oh = R8 == (le_row + base)
        ohb = oh.astype(bf16)
        cin = dot(ohb, U)
        tot = dot(ohb, ONES)
        off = dot(L, tot.astype(bf16))
        cum = cin + off
        if g == 0:
            cum0, off0, end0 = cum, off, off + tot
        rk = jnp.where(oh, cum, 0.0)
        for le in range(E_LOC):
            rank = rank + rk[le * 16:(le + 1) * 16]
    dropped = (rank > float(CAP)).astype(jnp.int32)
    dropped = jnp.where(rank == 0.0, 1, dropped)

    offT = off0.T
    endT = end0.T
    offT = jnp.concatenate([offT] * 4, axis=0)
    endT = jnp.concatenate([endT] * 4, axis=0)
    r5 = lax.broadcasted_iota(jnp.int32, (512, 128), 0)
    c5 = lax.broadcasted_iota(jnp.int32, (512, 128), 1)
    cf = (r5 & 63).astype(f32)
    sel = ((c5 >> 4) == (r5 >> 6)) & (offT <= cf) & (endT > cf)
    csel = dot(sel.astype(bf16), jnp.minimum(cum0, 128.0).astype(bf16))
    val = jnp.where(csel <= cf, 1.0, 0.0) + jnp.where(sel, ((c5 & 15) * 128).astype(f32), 0.0)
    tok = jnp.sum(val, axis=1, keepdims=True)
    tokd = jnp.where(c5 == (r5 & 63), tok, 0.0)
    tok8 = jnp.concatenate(
        [jnp.sum(tokd[le * 64:(le + 1) * 64], axis=0, keepdims=True) for le in range(E_LOC)],
        axis=0)
    tok8 = jnp.clip(tok8.astype(jnp.int32), 0, N_TOK - 1)
    cnt8 = jnp.concatenate([end0[le * 16 + 15:le * 16 + 16] for le in range(E_LOC)], axis=0)
    cnt8 = jnp.minimum(cnt8, float(CAP)).astype(jnp.int32)
    meta_v[0:16, :] = dropped
    meta_v[16:24, :] = tok8
    meta_v[24:32, :] = cnt8
    mcp = pltpu.make_async_copy(meta_v, meta_s, msem)
    mcp.start()
    mcp.wait()

    for e in range(E_LOC):
        def g_body(c, _, e=e):
            t = meta_s[16 + e, c]
            pltpu.make_async_copy(x_ref.at[pl.ds(t, 1)], xg.at[e, pl.ds(c, 1)], gsem.at[e]).start()
        lax.fori_loop(0, CAP, g_body, None, unroll=True)

    pl.semaphore_wait(bar, N_DEV - 1)

    nsend = 0
    for e in range(E_LOC):
        pltpu.make_async_copy(x_ref.at[pl.ds(0, 48)], xg.at[e, pl.ds(0, 48)], gsem.at[e]).wait()
        for _ in range(CAP - 48):
            pltpu.make_async_copy(x_ref.at[pl.ds(0, 1)], xg.at[e, pl.ds(0, 1)], gsem.at[e]).wait()
        wcps[e].wait()
        r = dot(xg[e].astype(bf16), wbuf[e].astype(bf16))
        u = pltpu.bitcast(r.astype(bf16).astype(f32), jnp.uint32)
        y[e] = u[:, H // 2:] | (u[:, :H // 2] >> 16)
        cnt = meta_s[24 + e, 0]
        nsend = nsend + cnt

        def s_body(c, _, e=e):
            t = meta_s[16 + e, c]
            pltpu.make_async_remote_copy(
                y.at[e, pl.ds(c, 1)], stage.at[pl.ds(t & (ROWS - 1), 1)], ssem, rsem,
                device_id=t >> 9, device_id_type=pl.DeviceIdType.LOGICAL).start()
        lax.fori_loop(0, cnt, s_body, None)

    for b in range(4):
        def z_body(j, _, b=b):
            @pl.when(meta_s[me * 4 + b, j] != 0)
            def _():
                pltpu.make_async_copy(zrow, stage.at[pl.ds(b * 128 + j, 1)], rsem).start()
        lax.fori_loop(0, 128, z_body, None, unroll=True)

    def w_body(c, _):
        pltpu.make_async_copy(y.at[0, pl.ds(0, 1)], y.at[0, pl.ds(0, 1)], ssem).wait()
    lax.fori_loop(0, nsend, w_body, None)
    pltpu.make_async_copy(stage, stage, rsem).wait()
    sv = stage[...]
    o_ref[:, :H // 2] = pltpu.bitcast(sv << 16, f32)
    o_ref[:, H // 2:] = pltpu.bitcast(sv & jnp.uint32(0xFFFF0000), f32)


def pallas_dist_moe_cap_ep_outshard_n2048_d512_e8_h1024_kernel(x, router_W, route_idx, expert_W):
    del router_W
    ri = route_idx.reshape(16, 128)
    return pl.pallas_call(
        _body,
        out_shape=jax.ShapeDtypeStruct((ROWS, H), jnp.float32),
        in_specs=[pl.BlockSpec(memory_space=pltpu.HBM)] * 3,
        out_specs=pl.BlockSpec(memory_space=pltpu.VMEM),
        scratch_shapes=[
            pltpu.VMEM((E_LOC, D, H), jnp.float32),
            pltpu.VMEM((E_LOC, CPAD, D), jnp.float32),
            pltpu.VMEM((E_LOC, CPAD, H // 2), jnp.uint32),
            pltpu.VMEM((16, 128), jnp.int32),
            pltpu.VMEM((32, 128), jnp.int32),
            pltpu.SMEM((32, 128), jnp.int32),
            pltpu.VMEM((1, H // 2), jnp.uint32),
            pltpu.VMEM((ROWS, H // 2), jnp.uint32),
            pltpu.SemaphoreType.DMA((E_LOC,)),
            pltpu.SemaphoreType.DMA((E_LOC,)),
            pltpu.SemaphoreType.DMA,
            pltpu.SemaphoreType.DMA,
            pltpu.SemaphoreType.DMA,
        ],
        compiler_params=pltpu.CompilerParams(collective_id=0, vmem_limit_bytes=64 * 1024 * 1024),
    )(x, ri, expert_W)
```
